```python
import numpy as np

kernel_name = "dist_sparse_attn_blocksparse_kvseq_b2_sq256_skv256_hq4_dh64"

def setup_inputs():
    x = np.random.randn(2, 256, 512).astype(np.float32)
    Wq = np.random.randn(512, 256).astype(np.float32) * 0.02
    K_ext = np.random.randn(2, 1024, 4, 64).astype(np.float32)
    V_ext = np.random.randn(2, 1024, 4, 64).astype(np.float32)
    Wo = np.random.randn(256, 512).astype(np.float32) * 0.02
    return {"x": x, "Wq": Wq, "K_ext": K_ext, "V_ext": V_ext, "Wo": Wo}

def reference(x, Wq, K_ext, V_ext, Wo):
    B, Sq, Skv, Hq, Dh = 2, 256, 1024, 4, 64
    Q = (x @ Wq).reshape(B, Sq, Hq, Dh)
    qb = (np.arange(Sq) // 64)[:, None]
    kb = (np.arange(Skv) // 64)[None, :]
    mask = (qb == kb) | (kb == 0) | ((qb + kb) % 3 == 0)
    scores = np.einsum('bihd,bjhd->bhij', Q, K_ext).astype(np.float32) * 0.125
    scores = np.where(mask[None, None, :, :], scores, -1e9)
    scores_max = scores.max(axis=-1, keepdims=True)
    w = np.exp(scores - scores_max)
    row_keep = mask.any(axis=1)
    w_sum = np.where(row_keep[None, None, :, None], w.sum(axis=-1, keepdims=True), 1.0)
    w = w / w_sum
    w = np.where(row_keep[None, None, :, None], w, 0.0)
    ctx = np.einsum('bhij,bjhd->bihd', w, V_ext).reshape(B, Sq, Hq * Dh)
    return ctx @ Wo
```

```python
import dataclasses
import functools

import jax
import jax.numpy as jnp
from jax import lax
from jax.experimental import pallas as pl
from jax.experimental.pallas import tpu as pltpu

B, SQ, D_MODEL = 2, 256, 512
HQ, DH = 4, 64
SKV_LOCAL = 256
BLK = 64
SCALE = 0.125
NEG = -1e9

TILE_QB = ((0, 3), (1, 2))
CLASSES = ((0, 0), (0, 1), (1, 1), (1, 0))
KEEPERS = ((0, 3), (0, 1), (1, 2), (2, 3))
MSG_ROWS = 33
NS = 2
SPLIT = ((2, 2), (2, 3), (1, 2))
PER_HEAD = ((2, 0),)


def _keep(qb, kb):
    return qb == kb or kb == 0 or (qb + kb) % 3 == 0


def _blocks(dev, tile):
    blocks = []
    for j in range(SKV_LOCAL // BLK):
        kb = dev * (SKV_LOCAL // BLK) + j
        lo, hi = (_keep(qb, kb) for qb in TILE_QB[tile])
        if lo or hi:
            blocks.append((j, lo, hi))
    return blocks


def _pair_up(blocks):
    ev = [b for b in blocks if b[0] % 2 == 0]
    od = [b for b in blocks if b[0] % 2 == 1]
    n = max(len(ev), len(od))
    return [(ev[i] if i < len(ev) else None, od[i] if i < len(od) else None)
            for i in range(n)]


def _plan(dev):
    nbrs = (dev ^ 1, 3 - dev)
    sent, kept = {}, {}
    for c, keepers in enumerate(KEEPERS):
        if dev in keepers:
            other = keepers[0] if keepers[1] == dev else keepers[1]
            child = nbrs[0] if nbrs[1] == other else nbrs[1]
            kept[c] = (other, child)
        else:
            sent[c] = nbrs[0] if nbrs[0] in keepers else nbrs[1]
    return sent, kept


SCHED = {
    0: dict(
        loads="w0 x2 x3 k10 k00 v10 v00 w1 k11 k01 v11 v01 x1 x0 o",
        prog="Q20 | Q30 | S20 S30 | V20 V30 D | Q21 Q31 | S21 S31 | V21 V31 D | "
             "Q10 Q11 | Q00 Q01 S10 | V10 D | S00 V00 D | S11 | S01 V01 D | V11 D | "
             "F000 F100 D | F001 F101 D | P00 P10 | F010 F110 D | F011 F111 D | "
             "P01 P11 | W6 | R300 R200 R301 R201 | P30 T20 | W | P31 T21",
    ),
    1: dict(
        loads="w0 x3 k00 v00 w1 k01 v01 x1 k10 v10 x2 k11 v11 o",
        prog="Q30 | S30 | V30 X00 D | Q31 | S31 | V31 X01 D | Q10 Q11 | S10 V10 D | "
             "Q20 Q21 | S11 S20 V11 D V20 M200 M201 D | S21 V21 M210 M211 D | "
             "G200 | G201 | F100 F101 D | G210 | G211 | F110 D | F111 D | "
             "P20 P21 P10 P11 | P00 | W4 | P30 | P01 P31 | W",
    ),
    2: dict(
        loads="k0000 v0000 k1000 v1000 k0001 v0001 k1001 v1001 k010 v010 k110 v110 "
              "w0 x3 x2 k001 k101 v001 v101 w1 k111 k011 v111 v011 o",
        prog="Y000 Y100 D | Y001 Y101 D | X01 X11 D | Q30 | Q20 | S30 S20 | "
             "V30 V20 M300 D | B212 M200 D Q21 Q31 | A210 A310 M301 M201 D S21 S31 | "
             "V21 V31 M310 M210 D | M311 D | M211 D | "
             "G200 G300 | G201 G301 | G210 G310 | G211 G311 | P20 P21 P30 P31 | "
             "P00 P10 | W | P01 P11",
    ),
    3: dict(
        loads="k10 v10 w0 x2 k11 w1 v11 x0 k00 v00 k01 v01 x3 o",
        prog="K10 D | U10 D J20 | q20 S20 v20 D | K11 D | q21 S21 | U11 D V21 Q00 D | "
             "J00 | S00 Q01 v00 D | S01 Q30 Q31 V01 D | "
             "S30 S31 V30 V31 M300 M301 M310 M311 D | "
             "G300 | G301 | F000 D | G310 | G311 | F001 D | F010 F011 D | "
             "P30 P31 P00 P01 | P10 | W4 | P20 | P11 P21 | W",
    ),
}


def pallas_dist_sparse_attn_blocksparse_kvseq_b2_sq256_skv256_hq4_dh64_kernel(
    x: jax.Array,
    Wq: jax.Array,
    K_ext: jax.Array,
    V_ext: jax.Array,
    Wo: jax.Array,
):
    f32, bf16 = jnp.float32, jnp.bfloat16
    kt = jnp.transpose(K_ext, (0, 2, 3, 1)).reshape(B, HQ * DH, SKV_LOCAL)
    vt = jnp.transpose(V_ext, (0, 2, 3, 1)).reshape(B, HQ * DH, SKV_LOCAL)

    def body(x_hbm, wq_hbm, kt_hbm, vt_hbm, wo_hbm, out_ref,
             xb, wqb, ktb, vtb, wob,
             snd1, rcv1, snd2, rcv2, kvs, kvr, ctx,
             lsem, ssem, rsem, ack):
        me = lax.axis_index("i")
        barrier = pltpu.get_barrier_semaphore()
        lo = lax.broadcasted_iota(jnp.int32, (1, 128), 1) < BLK

        def signal(sem, to):
            pl.semaphore_signal(sem, inc=1, device_id=(to,),
                                device_id_type=pl.DeviceIdType.MESH)

        def run(dev):
            sent, kept = _plan(dev)

            if dev != 2:
                for nbr in (dev ^ 1, 3 - dev):
                    signal(barrier, nbr)
            known = set()

            def ensure(to):
                if to in known:
                    return
                if dev in (0, 2):
                    pl.semaphore_wait(barrier, 2)
                    known.update((1, 3))
                else:
                    pl.semaphore_wait(barrier if to == 0 else ack, 1)
                    known.add(to)

            loads = {}
            started = []

            def start_load(keys, pairs):
                cps = []
                for src, dst in pairs:
                    cp = pltpu.make_async_copy(src, dst, lsem.at[len(started)])
                    cp.start()
                    started.append(cp)
                    cps.append(cp)
                for key in keys:
                    loads[key] = cps

            def need(key):
                if key not in loads:
                    need(key + "0")
                    need(key + "1")
                    return
                for cp in loads[key]:
                    cp.wait()
                loads[key].clear()

            for key in SCHED[dev]["loads"].split():
                a = [int(ch) for ch in key[1:]]
                if key[0] == "w":
                    start_load([key], [
                        (wq_hbm.at[pl.ds(i * 256, 256), pl.ds(a[0] * 128, 128)],
                         wqb.at[a[0], pl.ds(i * 256, 256)]) for i in range(2)])
                elif key[0] == "x":
                    t, b = CLASSES[a[0]]
                    start_load([key], [
                        (x_hbm.at[b, pl.ds(qb * BLK, BLK)],
                         xb.at[a[0], pl.ds(i * BLK, BLK)])
                        for i, qb in enumerate(TILE_QB[t])])
                elif key[0] == "o":
                    start_load([key], [(wo_hbm, wob)])
                else:
                    src, dst = (kt_hbm, ktb) if key[0] == "k" else (vt_hbm, vtb)
                    rows = pl.ds(a[1] * 128, 128)
                    if len(a) == 2:
                        start_load([key + "0", key + "1"],
                                   [(src.at[a[0], rows], dst.at[a[0], rows])])
                    else:
                        cols = pl.ds(a[2] * 128, 128)
                        if len(a) == 4:
                            rows = pl.ds((a[1] * 2 + a[3]) * DH, DH)
                        start_load([key], [(src.at[a[0], rows, cols],
                                            dst.at[a[0], rows, cols])])

            if dev == 2:
                ensure(1)
                signal(ack, 1)
                signal(ack, 3)

            def msg_idx(c, hp, hh):
                return c * 4 + hp * 2 + hh

            def remote(group, src, dst, idx, to):
                return pltpu.make_async_remote_copy(
                    src_ref=src, dst_ref=dst,
                    send_sem=ssem.at[group * 16 + idx],
                    recv_sem=rsem.at[group * 16 + idx],
                    device_id=(to,), device_id_type=pl.DeviceIdType.MESH)

            def nparts(c):
                return NS if CLASSES[c][0] == 1 else 1

            def part_rows(c, part):
                n = 32 // nparts(c)
                return 32 - (part + 1) * n, 32 - part * n

            def head_rows(c, part):
                n = DH // nparts(c)
                return part * n, (part + 1) * n

            def ctx_row(c, hp, hh):
                return (hp * 2 + hh if CLASSES[c][0] == 0 else hh * 2 + hp) * DH

            def p1(idx, to):
                return remote(0, snd1.at[idx - 8], rcv1.at[idx - 8], idx, to)

            def p2(c, hp, hh, part, to):
                idx = msg_idx(c, hp, hh)
                r0, r1 = part_rows(c, part)
                rows = pl.ds(r0, (MSG_ROWS if part == 0 else r1) - r0)
                return remote(1 + 2 * part, snd2.at[idx, rows], rcv2.at[idx, rows], idx, to)

            def p3(c, hp, hh, part, to):
                d0, d1 = head_rows(c, part)
                slot = ctx.at[c, pl.ds(ctx_row(c, hp, hh) + d0, d1 - d0)]
                return remote(2 + 2 * part, slot, slot, msg_idx(c, hp, hh), to)

            def pkv(c, hp, slot, to):
                idx = msg_idx(c, hp, slot)
                return remote(0, kvs.at[idx], kvr.at[idx], idx, to)

            def pkh(c, hp, hh, to):
                idx = msg_idx(c, hp, 0)
                rows = pl.ds(hh * DH, DH)
                return remote(0, kvs.at[idx, rows], kvr.at[idx, rows], idx + hh, to)

            def n_extra(c):
                if c in kept and CLASSES[c][0] == 0:
                    return len(_blocks(kept[c][1], 0))
                return 0

            def cols_of(c):
                return sorted({j // 2 for j, _, _ in _blocks(dev, CLASSES[c][0])})

            def pair_rows(hp):
                return slice(hp * 128, (hp + 1) * 128)

            def col(ref, b, rows, j):
                return ref[b, rows, (j // 2) * 128:(j // 2 + 1) * 128]

            def sel(ref, b, rows, lob, hib):
                if lob is None:
                    return col(ref, b, rows, hib[0]).astype(bf16)
                if hib is None or lob[0] // 2 == hib[0] // 2:
                    return col(ref, b, rows, lob[0]).astype(bf16)
                return jnp.where(lo, col(ref, b, rows, lob[0]),
                                 col(ref, b, rows, hib[0])).astype(bf16)

            def recip(v):
                r = pl.reciprocal(v, approx=True)
                return r * (2.0 - v * r)

            def pack(ref, idx, o, lse):
                ref[idx, 0:32, :] = pltpu.bitcast(o.astype(bf16), f32)
                ref[idx, 32:33, :] = lse

            Q, P, O, PRE, KS, KB = {}, {}, {}, {}, {}, {}
            pending, sends = [], []
            written, got3 = set(), set()

            def recv3(c, hp, hh):
                if c in sent and (c, hp, hh) not in got3:
                    got3.add((c, hp, hh))
                    for part in range(nparts(c)):
                        p3(c, hp, hh, part, sent[c]).wait_recv()

            def waits(op, a):
                if op == "W":
                    n = len(sends) - (a[0] if a else 0)
                    for cp in sends[:n]:
                        cp.wait_send()
                    del sends[:n]
                if op in "DW":
                    return
                c, hp = a[:2]
                b = CLASSES[c][1]
                if op in "QB":
                    need("w%d" % hp)
                    need("x%d" % c)
                for kv, users in (("k", "SXKJA"), ("v", "VXU")):
                    if op in users:
                        for cl in cols_of(c):
                            need("%s%d%d%d" % (kv, b, hp, cl))
                    if op == "Y":
                        need("%s%d%d%d%d" % (kv, b, hp, cols_of(c)[0], a[2]))
                if op == "S" and n_extra(c):
                    if (kept[c][1], hp) in PER_HEAD:
                        for hh in range(2):
                            pkh(c, hp, hh, kept[c][1]).wait_recv()
                    else:
                        pkv(c, hp, 0, kept[c][1]).wait_recv()
                if op == "V" and n_extra(c) == 2:
                    pkv(c, hp, 1, kept[c][1]).wait_recv()
                if op == "M":
                    p1(msg_idx(*a), kept[c][1]).wait_recv()
                if op == "F":
                    p2(*a, kept[c][0]).wait_recv()
                if op == "R":
                    recv3(*a)
                if op in "PT":
                    need("o")
                    for i in range(2):
                        recv3(c, *((hp, i) if CLASSES[c][0] == 0 else (i, hp)))
                if op in "XYKU" or (op == "V" and c in sent):
                    ensure(sent[c])
                if op == "M" or (op == "V" and n_extra(c)):
                    ensure(kept[c][0])
                if op == "F":
                    ensure(kept[c][1])

            def op_b(c, hp, n):
                PRE[c, hp] = (xb[c, :16 * n, :].astype(bf16), wqb[hp].astype(bf16))

            def flip(a):
                return jnp.concatenate(
                    [a[16 * i:16 * (i + 1)] for i in reversed(range(a.shape[0] // 16))],
                    axis=0)

            def op_q(c, hp, rev=False):
                if (c, hp) in PRE:
                    x0, w = PRE[c, hp]
                    xv = jnp.concatenate([x0, xb[c, x0.shape[0]:, :].astype(bf16)], axis=0)
                else:
                    xv, w = xb[c].astype(bf16), wqb[hp].astype(bf16)
                q = jnp.dot(flip(xv) if rev else xv, w, preferred_element_type=f32) * SCALE
                Q[c, hp] = flip(q) if rev else q

            def softmax_t(ks, tiles, qm, swap):
                def scores(k):
                    return lax.dot_general(k, qm, (((0,), (1,)), ((), ())),
                                           preferred_element_type=f32)
                ss = []
                for k, (lob, hib) in zip(ks, tiles):
                    if isinstance(k, tuple):
                        parts = [(scores(k[0][:, :BLK]), lob), (scores(k[1][:, :BLK]), hib)]
                    elif hib is None:
                        parts = [(scores(k[:, :BLK]), lob)]
                    else:
                        s = scores(k)
                        parts = [(s[:BLK], lob), (s[BLK:], hib)]
                    if (len(tiles) == 1 and lob is not None and hib is not None
                            and lob[1] != lob[2] and hib[1:] == (lob[2], lob[1])):
                        keep = lo if lob[1] != swap else ~lo
                        s = jnp.where(keep, parts[0][0], parts[1][0])
                        m = jnp.max(s, axis=0, keepdims=True)
                        p = jnp.exp(s - m)
                        return [[jnp.where(keep, p, 0.0), jnp.where(keep, 0.0, p)]], m, [p]
                    row = []
                    for sp, bk in parts:
                        if bk is not None and not (bk[1] and bk[2]):
                            sp = jnp.where(lo if bk[1] != swap else ~lo, sp, NEG)
                        row.append(None if bk is None else sp)
                    ss.append(row)
                m = functools.reduce(jnp.maximum, [s for r in ss for s in r if s is not None])
                m = jnp.max(m, axis=0, keepdims=True)
                ps = [[None if s is None else jnp.exp(s - m) for s in r] for r in ss]
                return ps, m, [p for r in ps for p in r if p is not None]

            def row_sum(flat):
                return jnp.sum(functools.reduce(jnp.add, flat), axis=0, keepdims=True)

            def to_tiles(ps):
                z = jnp.zeros((BLK, 128), f32)
                return [jnp.concatenate([z if p is None else p for p in r], axis=0).astype(bf16)
                        for r in ps]

            def split_tiles(i):
                return _pair_up([(blk[0], True, True) for blk in _blocks(dev, 1) if blk[1 + i]])

            def op_a(c, hp, i):
                KS[c, hp, i] = [sel(ktb, CLASSES[c][1], pair_rows(hp), *tl)
                                for tl in split_tiles(i)]

            def op_j(c, hp):
                t, b = CLASSES[c]
                KB[c, hp] = [(col(ktb, b, pair_rows(hp), lob[0]).astype(bf16),
                              pltpu.roll(col(ktb, b, pair_rows(hp), hib[0]), BLK, 1).astype(bf16))
                             for lob, hib in _pair_up(_blocks(dev, t))]

            def op_s(c, hp):
                t, b = CLASSES[c]
                q = Q[c, hp]
                res = []
                if (dev, c) in SPLIT:
                    for i in range(2):
                        qi = q[i * BLK:(i + 1) * BLK]
                        q0, q1 = jnp.where(lo, qi, 0.0), jnp.where(lo, 0.0, qi)
                        qm = jnp.concatenate([q1, q0] if i else [q0, q1], axis=0).astype(bf16)
                        if (c, hp, i) not in KS:
                            op_a(c, hp, i)
                        ps, m, live = softmax_t(KS[c, hp, i], split_tiles(i), qm, False)
                        res.append((to_tiles(ps), m, live))
                    P[c, hp] = res
                    return
                tiles = _pair_up(_blocks(dev, t))
                ks = list(KB[c, hp]) if (c, hp) in KB else [
                    sel(ktb, b, pair_rows(hp), *tl) for tl in tiles]
                if n_extra(c):
                    full = (0, True, True)
                    ks.append(kvr[msg_idx(c, hp, 0)])
                    tiles = tiles + [(full, None if n_extra(c) == 1 else full)]
                for hh in range(2):
                    swap = t == 1 and hh == 1
                    qq = jnp.concatenate([q[BLK:], q[:BLK]], axis=0) if swap else q
                    qm = jnp.where(~lo if hh else lo, qq, 0.0).astype(bf16)
                    ps, m, live = softmax_t(ks, tiles, qm, swap)
                    if n_extra(c) == 1:
                        ps[-1] = [None, ps[-1][0]]
                    res.append((to_tiles(ps), m, live))
                P[c, hp] = res

            def pv(vs, pb, halves=False):
                if halves:
                    n = vs[0].shape[0] // 2
                    return jnp.concatenate([pv([v[:n] for v in vs], pb),
                                            pv([v[n:] for v in vs], pb)], axis=0)
                return functools.reduce(jnp.add, [
                    jnp.dot(v[:, :p.shape[0]], p, preferred_element_type=f32)
                    for p, v in zip(pb, vs)])

            def op_v(c, hp, halves=False):
                t, b = CLASSES[c]
                outs = []
                if (dev, c) in SPLIT:
                    r = [pv([sel(vtb, b, pair_rows(hp), *tl) for tl in split_tiles(i)],
                            P[c, hp][i][0]) for i in range(2)]
                    (_, m0, l0), (_, m1, l1) = P[c, hp]
                    l0, l1 = row_sum(l0), row_sum(l1)
                    outs.append((jnp.where(lo, r[0][:DH], r[1][:DH]),
                                 jnp.where(lo, m0, m1), jnp.where(lo, l0, l1)))
                    outs.append((jnp.where(lo, r[1][DH:], r[0][DH:]),
                                 jnp.where(lo, m1, m0), jnp.where(lo, l1, l0)))
                else:
                    for hh in range(2):
                        pb, m, live = P[c, hp][hh]
                        rows = slice((hp * 2 + hh) * DH, (hp * 2 + hh + 1) * DH)
                        vs = [sel(vtb, b, rows, *tl) for tl in _pair_up(_blocks(dev, t))]
                        if n_extra(c):
                            vs.append(kvr[msg_idx(c, hp, n_extra(c) - 1),
                                          hh * DH:(hh + 1) * DH, :])
                        outs.append((pv(vs, pb, halves), m, row_sum(live)))
                for hh, (o, m, l) in enumerate(outs):
                    idx = msg_idx(c, hp, hh)
                    O[idx] = (o * recip(l), m + jnp.log(l))
                    if c in sent:
                        pending.append(((hh, -1), functools.partial(pack, snd1, idx - 8, *O[idx]),
                                        p1(idx, sent[c])))
                    elif n_extra(c):
                        pending.append(((hh, -1), functools.partial(pack, snd2, idx, *O[idx]),
                                        p2(c, hp, hh, 0, kept[c][0])))

            def op_x(c, hp, hh=None):
                t, b = CLASSES[c]
                (j, _, _), = _blocks(dev, t)
                rows = pair_rows(hp)
                if hh is not None:
                    rows = slice((hp * 2 + hh) * DH, (hp * 2 + hh + 1) * DH)
                k, v = col(ktb, b, rows, j), col(vtb, b, rows, j)
                if j % 2:
                    k = pltpu.roll(k, BLK, 1)
                else:
                    v = pltpu.roll(v, BLK, 1)
                kv = jnp.where(lo, k, v).astype(bf16)
                if hh is None:
                    kvs[msg_idx(c, hp, 0)] = kv
                    pending.append(((0, -1), None, pkv(c, hp, 0, sent[c])))
                else:
                    kvs[msg_idx(c, hp, 0), hh * DH:(hh + 1) * DH, :] = kv
                    pending.append(((0, -1), None, pkh(c, hp, hh, sent[c])))

            def ship_tile(ref, slot, c, hp):
                t, b = CLASSES[c]
                (tl,) = _pair_up(_blocks(dev, t))
                kvs[msg_idx(c, hp, slot)] = sel(ref, b, pair_rows(hp), *tl)
                pending.append(((0, -1), None, pkv(c, hp, slot, sent[c])))

            def weights(la, lb):
                mx = jnp.maximum(la, lb)
                wa = jnp.exp(la - mx)
                wb = jnp.exp(lb - mx)
                tot = wa + wb
                inv = recip(tot)
                return wa * inv, wb * inv, mx + jnp.log(tot)

            def op_m(c, hp, hh):
                idx = msg_idx(c, hp, hh)
                theirs = pltpu.bitcast(rcv1[idx - 8, 0:32, :], bf16).astype(f32)
                wa, wb, lse = weights(O[idx][1], rcv1[idx - 8, 32:33, :])
                o = wa * O[idx][0] + wb * theirs

                def store(part):
                    r0, r1 = part_rows(c, part)
                    d0, d1 = head_rows(c, part)
                    snd2[idx, r0:r1, :] = pltpu.bitcast(o[d0:d1].astype(bf16), f32)
                    if part == 0:
                        snd2[idx, 32:33, :] = lse

                nth = sum(1 for order, _, _ in pending if order[1:] == (0, c))
                for part in range(nparts(c)):
                    pending.append(((nth, part, c), functools.partial(store, part),
                                    p2(c, hp, hh, part, kept[c][0])))
                O[idx] = (o, lse)

            def op_f(c, hp, hh, part):
                idx = msg_idx(c, hp, hh)
                if part == 0:
                    wa, wb, _ = weights(O[idx][1], rcv2[idx, 32:33, :])
                    O[idx] = (wa * O[idx][0], wb)
                r0, r1 = part_rows(c, part)
                d0, d1 = head_rows(c, part)
                theirs = pltpu.bitcast(rcv2[idx, r0:r1, :], bf16).astype(f32)
                o = O[idx][0][d0:d1] + O[idx][1] * theirs
                base = ctx_row(c, hp, hh)
                ctx[c, base + d0:base + d1, :] = o.astype(bf16)
                pending.append(((0, -1), None, p3(c, hp, hh, part, kept[c][1])))

            def op_p(c, g, xpose=False):
                t, b = CLASSES[c]
                ct = ctx[c, g * 128:(g + 1) * 128, :]
                heads = (2 * g, 2 * g + 1) if t == 0 else (g, g + 2)
                w = jnp.concatenate([wob[h * DH:(h + 1) * DH, :] for h in heads],
                                    axis=0).astype(bf16)
                if xpose:
                    y = jnp.dot(ct.T, w, preferred_element_type=f32)
                else:
                    y = lax.dot_general(ct, w, (((0,), (0,)), ((), ())),
                                        preferred_element_type=f32)
                qbs = TILE_QB[t][::-1] if (t == 1 and g == 1) else TILE_QB[t]
                for i, qb in enumerate(qbs):
                    rows = pl.ds(qb * BLK, BLK)
                    yi = y[i * BLK:(i + 1) * BLK]
                    if c in written:
                        out_ref[b, rows, :] += yi
                    else:
                        out_ref[b, rows, :] = yi
                written.add(c)

            def op_d():
                for _, store, cp in sorted(pending, key=lambda it: it[0][:2]):
                    if store is not None:
                        store()
                    cp.start()
                    sends.append(cp)
                pending.clear()

            ops = dict(
                Q=op_q, q=functools.partial(op_q, rev=True), S=op_s,
                V=op_v, v=functools.partial(op_v, halves=True),
                A=op_a, B=op_b, J=op_j, X=op_x, Y=op_x,
                K=functools.partial(ship_tile, ktb, 0),
                U=functools.partial(ship_tile, vtb, 1),
                M=op_m, F=op_f, P=op_p, T=functools.partial(op_p, xpose=True),
                D=op_d, W=lambda *a: None, R=lambda *a: None)

            regions = []
            for region in SCHED[dev]["prog"].split("|"):
                tks = region.split()
                if tks[0][0] == "G":
                    regions += [["F%s%d" % (tk[1:], part), "D"]
                                for part in range(NS) for tk in tks]
                else:
                    regions.append([tk + "0" if tk[0] == "F" else tk for tk in tks])
            for region in regions:
                toks = [(tk[0], [int(ch) for ch in tk[1:]]) for tk in region]
                for op, a in toks:
                    waits(op.upper(), a)
                for op, a in toks:
                    ops[op](*a)
            assert not pending and not sends and not any(loads.values())

        for dev in (2, 1, 3, 0):
            pl.when(me == dev)(functools.partial(run, dev))

    params = dict(collective_id=0, disable_semaphore_checks=True,
                  fuse_transposed_lhs_in_matmul=True)
    fields = {f.name for f in dataclasses.fields(pltpu.CompilerParams)}
    return pl.pallas_call(
        body,
        out_shape=jax.ShapeDtypeStruct((B, SQ, D_MODEL), f32),
        in_specs=[pl.BlockSpec(memory_space=pl.ANY)] * 5,
        out_specs=pl.BlockSpec(memory_space=pltpu.VMEM),
        scratch_shapes=[
            pltpu.VMEM((4, 128, D_MODEL), f32),
            pltpu.VMEM((2, D_MODEL, 128), f32),
            pltpu.VMEM((B, HQ * DH, SKV_LOCAL), f32),
            pltpu.VMEM((B, HQ * DH, SKV_LOCAL), f32),
            pltpu.VMEM((HQ * DH, D_MODEL), f32),
            pltpu.VMEM((8, MSG_ROWS, 128), f32),
            pltpu.VMEM((8, MSG_ROWS, 128), f32),
            pltpu.VMEM((16, MSG_ROWS, 128), f32),
            pltpu.VMEM((16, MSG_ROWS, 128), f32),
            pltpu.VMEM((8, 128, 128), bf16),
            pltpu.VMEM((8, 128, 128), bf16),
            pltpu.VMEM((4, HQ * DH, 128), bf16),
            pltpu.SemaphoreType.DMA((32,)),
            pltpu.SemaphoreType.DMA((16 + 32 * NS,)),
            pltpu.SemaphoreType.DMA((16 + 32 * NS,)),
            pltpu.SemaphoreType.REGULAR,
        ],
        compiler_params=pltpu.CompilerParams(
            **{k: v for k, v in params.items() if k in fields}),
    )(x, Wq, kt, vt, Wo)
```

```python
import dataclasses
import functools

import jax
import jax.numpy as jnp
from jax import lax
from jax.experimental import pallas as pl
from jax.experimental.pallas import tpu as pltpu

B, SQ, D_MODEL = 2, 256, 512
HQ, DH = 4, 64
SKV_LOCAL = 256
BLK = 64
SCALE = 0.125
NEG = -1e9

TILE_QB = ((0, 3), (1, 2))
CLASSES = ((0, 0), (0, 1), (1, 1), (1, 0))
KEEPERS = ((0, 3), (0, 1), (1, 2), (2, 3))
MSG_ROWS = 33
NS = 4
SPLIT = ((2, 2), (2, 3), (1, 2))
CHUNKS = {(2, 0): (32, 32, 64), (3, 0): (64, 64)}
N_LOAD, N_SEND, N_RECV = 33, 72, 76


def _keep(qb, kb):
    return qb == kb or kb == 0 or (qb + kb) % 3 == 0


def _blocks(dev, tile):
    blocks = []
    for j in range(SKV_LOCAL // BLK):
        kb = dev * (SKV_LOCAL // BLK) + j
        lo, hi = (_keep(qb, kb) for qb in TILE_QB[tile])
        if lo or hi:
            blocks.append((j, lo, hi))
    return blocks


def _pair_up(blocks):
    ev = [b for b in blocks if b[0] % 2 == 0]
    od = [b for b in blocks if b[0] % 2 == 1]
    n = max(len(ev), len(od))
    return [(ev[i] if i < len(ev) else None, od[i] if i < len(od) else None)
            for i in range(n)]


def _chunk(dev, hp, i):
    sizes = CHUNKS[dev, hp]
    return sum(sizes[:i]), sizes[i]


def _plan(dev):
    nbrs = (dev ^ 1, 3 - dev)
    sent, kept = {}, {}
    for c, keepers in enumerate(KEEPERS):
        if dev in keepers:
            other = keepers[0] if keepers[1] == dev else keepers[1]
            child = nbrs[0] if nbrs[1] == other else nbrs[1]
            kept[c] = (other, child)
        else:
            sent[c] = nbrs[0] if nbrs[0] in keepers else nbrs[1]
    return sent, kept


SCHED = {
    0: dict(
        loads="w0 x0 x1 w1 x2 x3 k10 k00 v10 v00 k11 k01 v11 v01 o",
        prog="Q00 | Q10 | Z00 Z10 D | Q01 Q11 Z01 Z11 D | Q20 Q21 | Q30 Q31 | "
             "S20 S30 | V20 V30 D | S21 S31 | V21 V31 D | "
             "S10 S11 | S00 V00 D | V10 D | S01 V01 D | V11 D | "
             "F000 F100 D | F001 F101 D | P00 P10 | F010 F110 D | F011 F111 D | "
             "P01 P11 | W9 | R300 R200 R301 R201 W5 | P30 T20 | W2 | P31 T21 | W",
    ),
    1: dict(
        loads="w0 x31 x30 k00 v00 w1 k01 v01 k10 v10 x2 k11 v11 o",
        prog="H30 | Q30 | S30 | v30 X00 D | Q31 | S31 | V31 X01 D | I10 S10 v10 D | "
             "Q20 Q21 | I11 S11 v11 D | S20 S21 V20 V21 M200 M201 D | M210 D | "
             "G200 | M211 D | G201 | G210 | G211 | F100 F101 D | F110 D | F111 D | "
             "P20 P21 P10 P11 | P00 | W4 | P30 | P01 P31 | W",
    ),
    2: dict(
        loads="k0000 v0000 k1000 v1000 k0001 v0001 k1001 v1001 "
              "k0002 v0002 k1002 v1002 k010 v010 k110 v110 "
              "w0 x3 x2 k001 k101 v001 v101 w1 k111 k011 v111 v011 o",
        prog="Y000 Y100 D | Y001 Y101 D | Y002 Y102 D | X01 X11 D | Q30 | Q20 | "
             "S30 S20 | V30 V20 M300 D | B212 M200 D Q21 Q31 | "
             "A210 A310 M301 M201 D S21 S31 | V21 V31 M310 M210 D | M311 D | M211 D | "
             "G200 G300 | G201 G301 | G210 G310 | G211 G311 | P20 P21 P30 P31 | "
             "P00 P10 | W | P01 P11",
    ),
    3: dict(
        loads="k1020 k1021 k11 w0 x21 x20 v10 w1 v11 k00 v00 k01 x3 v01 o",
        prog="K100 D | K101 D | K11 D J20 J21 | H20 | q20 S20 | U10 D v20 D | "
             "q21 S21 | U11 D V21 D | J00 | I00 S00 v00 D | J01 Q30 Q31 | "
             "I01 S01 v01 D | S30 S31 V30 V31 M300 M301 D | M310 D | "
             "G300 | M311 D | G301 | G310 | G311 | F000 F001 D | F010 F011 D | "
             "P30 P31 P00 P01 | P10 | W4 | P20 | P11 P21 | W",
    ),
}


def pallas_dist_sparse_attn_blocksparse_kvseq_b2_sq256_skv256_hq4_dh64_kernel(
    x: jax.Array,
    Wq: jax.Array,
    K_ext: jax.Array,
    V_ext: jax.Array,
    Wo: jax.Array,
):
    f32, bf16 = jnp.float32, jnp.bfloat16
    kt = jnp.transpose(K_ext, (0, 2, 3, 1)).reshape(B, HQ * DH, SKV_LOCAL)
    vt = jnp.transpose(V_ext, (0, 2, 3, 1)).reshape(B, HQ * DH, SKV_LOCAL)

    def body(x_hbm, wq_hbm, kt_hbm, vt_hbm, wo_hbm, out_ref,
             xb, wqb, ktb, vtb, wob,
             snd1, rcv1, snd2, rcv2, kvs, kvr, ctx,
             lsem, ssem, rsem, ack):
        me = lax.axis_index("i")
        barrier = pltpu.get_barrier_semaphore()
        lo = lax.broadcasted_iota(jnp.int32, (1, 128), 1) < BLK

        def signal(sem, to):
            pl.semaphore_signal(sem, inc=1, device_id=(to,),
                                device_id_type=pl.DeviceIdType.MESH)

        recv_ids = {}

        def run(dev):
            sent, kept = _plan(dev)

            if dev != 2:
                for nbr in (dev ^ 1, 3 - dev):
                    signal(barrier, nbr)
            known = set()

            def ensure(to):
                if to in known:
                    return
                if dev in (0, 2):
                    pl.semaphore_wait(barrier, 2)
                    known.update((1, 3))
                else:
                    pl.semaphore_wait(barrier if to == 0 else ack, 1)
                    known.add(to)

            loads = {}
            started = []

            def start_load(keys, pairs):
                cps = []
                for src, dst in pairs:
                    cp = pltpu.make_async_copy(src, dst, lsem.at[len(started)])
                    cp.start()
                    started.append(cp)
                    cps.append(cp)
                for key in keys:
                    loads[key] = cps

            def need(key):
                if key not in loads:
                    subs = [k for k in loads if k[:-1] == key]
                    assert subs, key
                    for sub in subs:
                        need(sub)
                    return
                for cp in loads[key]:
                    cp.wait()
                loads[key].clear()

            for key in SCHED[dev]["loads"].split():
                a = [int(ch) for ch in key[1:]]
                if key[0] == "w":
                    start_load([key], [
                        (wq_hbm.at[pl.ds(i * 256, 256), pl.ds(a[0] * 128, 128)],
                         wqb.at[a[0], pl.ds(i * 256, 256)]) for i in range(2)])
                elif key[0] == "x":
                    t, b = CLASSES[a[0]]
                    for i in a[1:] or range(2):
                        start_load(["x%d%d" % (a[0], i)],
                                   [(x_hbm.at[b, pl.ds(TILE_QB[t][i] * BLK, BLK)],
                                     xb.at[a[0], pl.ds(i * BLK, BLK)])])
                elif key[0] == "o":
                    start_load([key], [(wo_hbm, wob)])
                else:
                    src, dst = (kt_hbm, ktb) if key[0] == "k" else (vt_hbm, vtb)
                    rows = pl.ds(a[1] * 128, 128)
                    if len(a) == 2:
                        start_load([key + "0", key + "1"],
                                   [(src.at[a[0], rows], dst.at[a[0], rows])])
                    else:
                        cols = pl.ds(a[2] * 128, 128)
                        keys = [key]
                        if len(a) == 4:
                            r0, n = _chunk(dev, a[1], a[3])
                            rows = pl.ds(a[1] * 128 + r0, n)
                            if a[2] == 2:
                                cols = pl.ds(0, 256)
                                keys = [key[:3] + str(cl) + key[4] for cl in range(2)]
                        start_load(keys, [(src.at[a[0], rows, cols],
                                           dst.at[a[0], rows, cols])])

            if dev == 2:
                ensure(1)
                signal(ack, 1)
                signal(ack, 3)

            def msg_idx(c, hp, hh):
                return c * 4 + hp * 2 + hh

            send_ids = {}

            def recv_sem(key):
                return rsem.at[recv_ids.setdefault(key, len(recv_ids))]

            def remote(key, src, dst, to, recv_key=None):
                sid = 0 if to is None else send_ids.setdefault(key, len(send_ids))
                return pltpu.make_async_remote_copy(
                    src_ref=src, dst_ref=dst, send_sem=ssem.at[sid],
                    recv_sem=recv_sem(recv_key or key),
                    device_id=(dev if to is None else to,),
                    device_id_type=pl.DeviceIdType.MESH)

            def nparts(c):
                return NS if CLASSES[c][0] == 1 else 1

            def part_rows(c, part):
                n = 32 // nparts(c)
                return 32 - (part + 1) * n, 32 - part * n

            def head_rows(c, part):
                n = DH // nparts(c)
                return part * n, (part + 1) * n

            def ctx_row(c, hp, hh):
                return (hp * 2 + hh if CLASSES[c][0] == 0 else hh * 2 + hp) * DH

            def p1(idx, to=None):
                return remote(("p1", idx), snd1.at[idx - 8], rcv1.at[idx - 8], to)

            def p2(c, hp, hh, part, to=None):
                idx = msg_idx(c, hp, hh)
                r0, r1 = part_rows(c, part)
                rows = pl.ds(r0, (MSG_ROWS if part == 0 else r1) - r0)
                return remote(("p2", idx, part), snd2.at[idx, rows], rcv2.at[idx, rows], to)

            def p3(c, hp, hh, part, to):
                d0, d1 = head_rows(c, part)
                slot = ctx.at[c, pl.ds(ctx_row(c, hp, hh) + d0, d1 - d0)]
                idx = msg_idx(c, hp, hh)
                return remote(("p3", idx, part), slot, slot, to, ("p3", idx))

            def pkv(c, hp, slot, to=None):
                idx = msg_idx(c, hp, slot)
                return remote(("kv", idx, 0), kvs.at[idx], kvr.at[idx], to)

            def pkh(c, hp, i, sender, to=None):
                idx = msg_idx(c, hp, 0)
                rows = pl.ds(*_chunk(sender, hp, i))
                return remote(("kv", idx, i), kvs.at[idx, rows], kvr.at[idx, rows], to)

            def n_extra(c):
                if c in kept and CLASSES[c][0] == 0:
                    return len(_blocks(kept[c][1], 0))
                return 0

            def cols_of(c):
                return sorted({j // 2 for j, _, _ in _blocks(dev, CLASSES[c][0])})

            def pair_rows(hp):
                return slice(hp * 128, (hp + 1) * 128)

            def col(ref, b, rows, j):
                return ref[b, rows, (j // 2) * 128:(j // 2 + 1) * 128]

            def sel(ref, b, rows, lob, hib):
                if lob is None:
                    return col(ref, b, rows, hib[0]).astype(bf16)
                if hib is None or lob[0] // 2 == hib[0] // 2:
                    return col(ref, b, rows, lob[0]).astype(bf16)
                return jnp.where(lo, col(ref, b, rows, lob[0]),
                                 col(ref, b, rows, hib[0])).astype(bf16)

            def recip(v):
                r = pl.reciprocal(v, approx=True)
                return r * (2.0 - v * r)

            def pack(ref, idx, o, lse):
                ref[idx, 0:32, :] = pltpu.bitcast(o.astype(bf16), f32)
                ref[idx, 32:33, :] = lse

            Q, P, O, PRE, KS, KB = {}, {}, {}, {}, {}, {}
            pending, sends = [], []
            written, got3 = set(), set()

            def recv3(c, hp, hh):
                if c in sent and (c, hp, hh) not in got3:
                    got3.add((c, hp, hh))
                    slot = ctx.at[c, pl.ds(ctx_row(c, hp, hh), DH)]
                    pltpu.make_async_copy(
                        slot, slot, recv_sem(("p3", msg_idx(c, hp, hh)))).wait()

            def waits(op, a):
                if op == "W":
                    n = len(sends) - (a[0] if a else 0)
                    for cp in sends[:n]:
                        cp.wait_send()
                    del sends[:n]
                if op in "DW":
                    return
                c, hp = a[:2]
                b = CLASSES[c][1]
                if op in "QBH":
                    need("w%d" % hp)
                    need("x%d1" % c if op == "H" else "x%d" % c)
                for kv, users in (("k", "SXKJA"), ("v", "VXU")):
                    if op in users:
                        for cl in cols_of(c):
                            need("%s%d%d%d" % (kv, b, hp, cl)
                                 + (str(a[2]) if op == "K" and len(a) == 3 else ""))
                    if op == "Y":
                        need("%s%d%d%d%d" % (kv, b, hp, cols_of(c)[0], a[2]))
                if op == "S" and n_extra(c):
                    if (kept[c][1], hp) in CHUNKS:
                        for i in range(len(CHUNKS[kept[c][1], hp])):
                            pkh(c, hp, i, kept[c][1]).wait_recv()
                    else:
                        pkv(c, hp, 0).wait_recv()
                if op == "I" or (op == "V" and n_extra(c) == 2):
                    pkv(c, hp, 1).wait_recv()
                if op == "M":
                    p1(msg_idx(*a)).wait_recv()
                if op == "F":
                    p2(*a).wait_recv()
                if op == "R":
                    recv3(*a)
                if op in "PT":
                    need("o")
                    for i in range(2):
                        recv3(c, *((hp, i) if CLASSES[c][0] == 0 else (i, hp)))
                if op in "XYKU" or (op == "V" and c in sent):
                    ensure(sent[c])
                if op in "MZ" or (op == "V" and n_extra(c)):
                    ensure(kept[c][0])
                if op == "F":
                    ensure(kept[c][1])

            def op_b(c, hp, n):
                PRE[c, hp] = (xb[c, :16 * n, :].astype(bf16), wqb[hp].astype(bf16))

            def flip(a):
                return jnp.concatenate(
                    [a[16 * i:16 * (i + 1)] for i in reversed(range(a.shape[0] // 16))],
                    axis=0)

            def op_h(c, hp):
                Q[c, hp] = jnp.dot(xb[c, BLK:, :].astype(bf16), wqb[hp].astype(bf16),
                                   preferred_element_type=f32) * SCALE

            def op_q(c, hp, rev=False):
                if (c, hp) in Q:
                    q = flip(jnp.dot(flip(xb[c, :BLK, :].astype(bf16)), wqb[hp].astype(bf16),
                                     preferred_element_type=f32) * SCALE)
                    Q[c, hp] = jnp.concatenate([q, Q[c, hp]], axis=0)
                    return
                if (c, hp) in PRE:
                    x0, w = PRE[c, hp]
                    xv = jnp.concatenate([x0, xb[c, x0.shape[0]:, :].astype(bf16)], axis=0)
                else:
                    xv, w = xb[c].astype(bf16), wqb[hp].astype(bf16)
                q = jnp.dot(flip(xv) if rev else xv, w, preferred_element_type=f32) * SCALE
                Q[c, hp] = flip(q) if rev else q

            def op_z(c, hp):
                kvs[msg_idx(c, hp, 1)] = Q[c, hp].astype(bf16)
                pending.append(((0, -1), None, pkv(c, hp, 1, kept[c][0])))

            def op_i(c, hp):
                Q[c, hp] = kvr[msg_idx(c, hp, 1)].astype(f32)

            def softmax_t(ks, tiles, qm, swap):
                def scores(k):
                    return lax.dot_general(k, qm, (((0,), (1,)), ((), ())),
                                           preferred_element_type=f32)
                ss = []
                for k, (lob, hib) in zip(ks, tiles):
                    if isinstance(k, tuple):
                        parts = [(scores(k[0][:, :BLK]), lob), (scores(k[1][:, :BLK]), hib)]
                    elif hib is None:
                        parts = [(scores(k[:, :BLK]), lob)]
                    else:
                        s = scores(k)
                        parts = [(s[:BLK], lob), (s[BLK:], hib)]
                    if (len(tiles) == 1 and lob is not None and hib is not None
                            and lob[1] != lob[2] and hib[1:] == (lob[2], lob[1])):
                        keep = lo if lob[1] != swap else ~lo
                        s = jnp.where(keep, parts[0][0], parts[1][0])
                        m = jnp.max(s, axis=0, keepdims=True)
                        p = jnp.exp(s - m)
                        return [[jnp.where(keep, p, 0.0), jnp.where(keep, 0.0, p)]], m, [p]
                    row = []
                    for sp, bk in parts:
                        if bk is not None and not (bk[1] and bk[2]):
                            sp = jnp.where(lo if bk[1] != swap else ~lo, sp, NEG)
                        row.append(None if bk is None else sp)
                    ss.append(row)
                m = functools.reduce(jnp.maximum, [s for r in ss for s in r if s is not None])
                m = jnp.max(m, axis=0, keepdims=True)
                ps = [[None if s is None else jnp.exp(s - m) for s in r] for r in ss]
                return ps, m, [p for r in ps for p in r if p is not None]

            def row_sum(flat):
                return jnp.sum(functools.reduce(jnp.add, flat), axis=0, keepdims=True)

            def to_tiles(ps):
                z = jnp.zeros((BLK, 128), f32)
                return [jnp.concatenate([z if p is None else p for p in r], axis=0).astype(bf16)
                        for r in ps]

            def split_tiles(i):
                return _pair_up([(blk[0], True, True) for blk in _blocks(dev, 1) if blk[1 + i]])

            def op_a(c, hp, i):
                KS[c, hp, i] = [sel(ktb, CLASSES[c][1], pair_rows(hp), *tl)
                                for tl in split_tiles(i)]

            def op_j(c, hp):
                t, b = CLASSES[c]
                KB[c, hp] = [(col(ktb, b, pair_rows(hp), lob[0]).astype(bf16),
                              pltpu.roll(col(ktb, b, pair_rows(hp), hib[0]), BLK, 1).astype(bf16))
                             for lob, hib in _pair_up(_blocks(dev, t))]

            def op_s(c, hp):
                t, b = CLASSES[c]
                q = Q[c, hp]
                res = []
                if (dev, c) in SPLIT:
                    for i in range(2):
                        qi = q[i * BLK:(i + 1) * BLK]
                        q0, q1 = jnp.where(lo, qi, 0.0), jnp.where(lo, 0.0, qi)
                        qm = jnp.concatenate([q1, q0] if i else [q0, q1], axis=0).astype(bf16)
                        if (c, hp, i) not in KS:
                            op_a(c, hp, i)
                        ps, m, live = softmax_t(KS[c, hp, i], split_tiles(i), qm, False)
                        res.append((to_tiles(ps), m, live))
                    P[c, hp] = res
                    return
                tiles = _pair_up(_blocks(dev, t))
                ks = list(KB[c, hp]) if (c, hp) in KB else [
                    sel(ktb, b, pair_rows(hp), *tl) for tl in tiles]
                if n_extra(c):
                    full = (0, True, True)
                    ks.append(kvr[msg_idx(c, hp, 0)])
                    tiles = tiles + [(full, None if n_extra(c) == 1 else full)]
                for hh in range(2):
                    swap = t == 1 and hh == 1
                    qq = jnp.concatenate([q[BLK:], q[:BLK]], axis=0) if swap else q
                    qm = jnp.where(~lo if hh else lo, qq, 0.0).astype(bf16)
                    ps, m, live = softmax_t(ks, tiles, qm, swap)
                    if n_extra(c) == 1:
                        ps[-1] = [None, ps[-1][0]]
                    res.append((to_tiles(ps), m, live))
                P[c, hp] = res

            def pv(vs, pb, halves=False):
                if halves:
                    n = vs[0].shape[0] // 2
                    return jnp.concatenate([pv([v[:n] for v in vs], pb),
                                            pv([v[n:] for v in vs], pb)], axis=0)
                return functools.reduce(jnp.add, [
                    jnp.dot(v[:, :p.shape[0]], p, preferred_element_type=f32)
                    for p, v in zip(pb, vs)])

            def op_v(c, hp, halves=False):
                t, b = CLASSES[c]
                outs = []
                if (dev, c) in SPLIT:
                    r = [pv([sel(vtb, b, pair_rows(hp), *tl) for tl in split_tiles(i)],
                            P[c, hp][i][0]) for i in range(2)]
                    (_, m0, l0), (_, m1, l1) = P[c, hp]
                    l0, l1 = row_sum(l0), row_sum(l1)
                    outs.append((jnp.where(lo, r[0][:DH], r[1][:DH]),
                                 jnp.where(lo, m0, m1), jnp.where(lo, l0, l1)))
                    outs.append((jnp.where(lo, r[1][DH:], r[0][DH:]),
                                 jnp.where(lo, m1, m0), jnp.where(lo, l1, l0)))
                else:
                    for hh in range(2):
                        pb, m, live = P[c, hp][hh]
                        rows = slice((hp * 2 + hh) * DH, (hp * 2 + hh + 1) * DH)
                        vs = [sel(vtb, b, rows, *tl) for tl in _pair_up(_blocks(dev, t))]
                        if n_extra(c):
                            vs.append(kvr[msg_idx(c, hp, n_extra(c) - 1),
                                          hh * DH:(hh + 1) * DH, :])
                        outs.append((pv(vs, pb, halves), m, row_sum(live)))
                for hh, (o, m, l) in enumerate(outs):
                    idx = msg_idx(c, hp, hh)
                    O[idx] = (o * recip(l), m + jnp.log(l))
                    if c in sent:
                        pending.append(((hh, -1), functools.partial(pack, snd1, idx - 8, *O[idx]),
                                        p1(idx, sent[c])))
                    elif n_extra(c):
                        pending.append(((hh, -1), functools.partial(pack, snd2, idx, *O[idx]),
                                        p2(c, hp, hh, 0, kept[c][0])))

            def op_x(c, hp, i=None):
                t, b = CLASSES[c]
                (j, _, _), = _blocks(dev, t)
                rows = pair_rows(hp)
                if i is not None:
                    r0, n = _chunk(dev, hp, i)
                    rows = slice(hp * 128 + r0, hp * 128 + r0 + n)
                k, v = col(ktb, b, rows, j), col(vtb, b, rows, j)
                if j % 2:
                    k = pltpu.roll(k, BLK, 1)
                else:
                    v = pltpu.roll(v, BLK, 1)
                kv = jnp.where(lo, k, v).astype(bf16)
                if i is None:
                    kvs[msg_idx(c, hp, 0)] = kv
                    pending.append(((0, -1), None, pkv(c, hp, 0, sent[c])))
                else:
                    kvs[msg_idx(c, hp, 0), r0:r0 + n, :] = kv
                    pending.append(((0, -1), None, pkh(c, hp, i, dev, sent[c])))

            def ship_tile(ref, slot, c, hp, i=None):
                t, b = CLASSES[c]
                (tl,) = _pair_up(_blocks(dev, t))
                if i is not None:
                    r0, n = _chunk(dev, hp, i)
                    kvs[msg_idx(c, hp, 0), r0:r0 + n, :] = sel(
                        ref, b, slice(hp * 128 + r0, hp * 128 + r0 + n), *tl)
                    pending.append(((0, -1), None, pkh(c, hp, i, dev, sent[c])))
                    return
                kvs[msg_idx(c, hp, slot)] = sel(ref, b, pair_rows(hp), *tl)
                pending.append(((0, -1), None, pkv(c, hp, slot, sent[c])))

            def weights(la, lb):
                mx = jnp.maximum(la, lb)
                wa = jnp.exp(la - mx)
                wb = jnp.exp(lb - mx)
                tot = wa + wb
                inv = recip(tot)
                return wa * inv, wb * inv, mx + jnp.log(tot)

            def op_m(c, hp, hh):
                idx = msg_idx(c, hp, hh)
                theirs = pltpu.bitcast(rcv1[idx - 8, 0:32, :], bf16).astype(f32)
                wa, wb, lse = weights(O[idx][1], rcv1[idx - 8, 32:33, :])
                o = wa * O[idx][0] + wb * theirs

                def store(part):
                    r0, r1 = part_rows(c, part)
                    d0, d1 = head_rows(c, part)
                    snd2[idx, r0:r1, :] = pltpu.bitcast(o[d0:d1].astype(bf16), f32)
                    if part == 0:
                        snd2[idx, 32:33, :] = lse

                nth = sum(1 for order, _, _ in pending if order[1:] == (0, c))
                for part in range(nparts(c)):
                    pending.append(((nth, part, c), functools.partial(store, part),
                                    p2(c, hp, hh, part, kept[c][0])))
                O[idx] = (o, lse)

            def op_f(c, hp, hh, part):
                idx = msg_idx(c, hp, hh)
                if part == 0:
                    wa, wb, _ = weights(O[idx][1], rcv2[idx, 32:33, :])
                    O[idx] = (wa * O[idx][0], wb)
                r0, r1 = part_rows(c, part)
                d0, d1 = head_rows(c, part)
                theirs = pltpu.bitcast(rcv2[idx, r0:r1, :], bf16).astype(f32)
                o = O[idx][0][d0:d1] + O[idx][1] * theirs
                base = ctx_row(c, hp, hh)
                ctx[c, base + d0:base + d1, :] = o.astype(bf16)
                pending.append(((0, -1), None, p3(c, hp, hh, part, kept[c][1])))

            def op_p(c, g, xpose=False):
                t, b = CLASSES[c]
                ct = ctx[c, g * 128:(g + 1) * 128, :]
                heads = (2 * g, 2 * g + 1) if t == 0 else (g, g + 2)
                w = jnp.concatenate([wob[h * DH:(h + 1) * DH, :] for h in heads],
                                    axis=0).astype(bf16)
                if xpose:
                    y = jnp.dot(ct.T, w, preferred_element_type=f32)
                else:
                    y = lax.dot_general(ct, w, (((0,), (0,)), ((), ())),
                                        preferred_element_type=f32)
                qbs = TILE_QB[t][::-1] if (t == 1 and g == 1) else TILE_QB[t]
                for i, qb in enumerate(qbs):
                    rows = pl.ds(qb * BLK, BLK)
                    yi = y[i * BLK:(i + 1) * BLK]
                    if c in written:
                        out_ref[b, rows, :] += yi
                    else:
                        out_ref[b, rows, :] = yi
                written.add(c)

            def op_d():
                for _, store, cp in sorted(pending, key=lambda it: it[0][:2]):
                    if store is not None:
                        store()
                    cp.start()
                    sends.append(cp)
                pending.clear()

            ops = dict(
                Q=op_q, q=functools.partial(op_q, rev=True), S=op_s,
                V=op_v, v=functools.partial(op_v, halves=True),
                A=op_a, B=op_b, H=op_h, Z=op_z, I=op_i, J=op_j, X=op_x, Y=op_x,
                K=functools.partial(ship_tile, ktb, 0),
                U=functools.partial(ship_tile, vtb, 1),
                M=op_m, F=op_f, P=op_p, T=functools.partial(op_p, xpose=True),
                D=op_d, W=lambda *a: None, R=lambda *a: None)

            regions = []
            for region in SCHED[dev]["prog"].split("|"):
                tks = region.split()
                if tks[0][0] == "G":
                    regions += [["F%s%d" % (tk[1:], part), "D"]
                                for part in range(NS) for tk in tks]
                else:
                    regions.append([tk + "0" if tk[0] == "F" else tk for tk in tks])
            for region in regions:
                toks = [(tk[0], [int(ch) for ch in tk[1:]]) for tk in region]
                for op, a in toks:
                    waits(op.upper(), a)
                for op, a in toks:
                    ops[op](*a)
            assert not pending and not sends and not any(loads.values())
            assert len(started) <= N_LOAD and len(send_ids) <= N_SEND
            assert len(recv_ids) <= N_RECV

        for dev in (2, 1, 3, 0):
            pl.when(me == dev)(functools.partial(run, dev))

    params = dict(collective_id=0, disable_semaphore_checks=True,
                  fuse_transposed_lhs_in_matmul=True)
    fields = {f.name for f in dataclasses.fields(pltpu.CompilerParams)}
    return pl.pallas_call(
        body,
        out_shape=jax.ShapeDtypeStruct((B, SQ, D_MODEL), f32),
        in_specs=[pl.BlockSpec(memory_space=pl.ANY)] * 5,
        out_specs=pl.BlockSpec(memory_space=pltpu.VMEM),
        scratch_shapes=[
            pltpu.VMEM((4, 128, D_MODEL), f32),
            pltpu.VMEM((2, D_MODEL, 128), f32),
            pltpu.VMEM((B, HQ * DH, SKV_LOCAL), f32),
            pltpu.VMEM((B, HQ * DH, SKV_LOCAL), f32),
            pltpu.VMEM((HQ * DH, D_MODEL), f32),
            pltpu.VMEM((8, MSG_ROWS, 128), f32),
            pltpu.VMEM((8, MSG_ROWS, 128), f32),
            pltpu.VMEM((16, MSG_ROWS, 128), f32),
            pltpu.VMEM((16, MSG_ROWS, 128), f32),
            pltpu.VMEM((8, 128, 128), bf16),
            pltpu.VMEM((8, 128, 128), bf16),
            pltpu.VMEM((4, HQ * DH, 128), bf16),
            pltpu.SemaphoreType.DMA((N_LOAD,)),
            pltpu.SemaphoreType.DMA((N_SEND,)),
            pltpu.SemaphoreType.DMA((N_RECV,)),
            pltpu.SemaphoreType.REGULAR,
        ],
        compiler_params=pltpu.CompilerParams(
            **{k: v for k, v in params.items() if k in fields}),
    )(x, Wq, kt, vt, Wo)
```
